```python
import numpy as np

kernel_name = "dist_ar_xy_y_m1024_n512"

def setup_inputs():
    return {"x": np.random.randn(2048, 512).astype(np.float32)}

def reference(x: np.ndarray) -> np.ndarray:
    return x.reshape(2, 1024, 512).sum(axis=0)
```

```python
import jax
import jax.numpy as jnp
from jax import lax
from jax.experimental import pallas as pl
from jax.experimental.pallas import tpu as pltpu

M, N = 1024, 512
HALF = M // 2
ROWS = 16
EXTRA = 2
MESH = pl.DeviceIdType.MESH


def pallas_dist_ar_xy_y_m1024_n512_kernel(
x: jax.Array,
):
    n_half = HALF // ROWS
    forwarded = list(range(EXTRA, n_half))
    order = forwarded + list(range(n_half, n_half + EXTRA)) + list(range(EXTRA))
    n = len(order)

    def kernel_body(x_ref, o_ref, xbuf, sbuf, rbuf, ld_sems, y_send, y_recv,
                    x_send, x_recv, x_ready):
        mx, my = lax.axis_index("x"), lax.axis_index("y")
        y_nbr, x_nbr = (mx, 1 - my), (1 - mx, my)

        def rows(b):
            half = mx if b < n_half else 1 - mx
            return pl.ds(pl.multiple_of(half * HALF + (b % n_half) * ROWS, ROWS), ROWS)

        loads = [pltpu.make_async_copy(x_ref.at[rows(b)], xbuf.at[i], ld_sems.at[i])
                 for i, b in enumerate(order)]
        loads[0].start()
        barrier = pltpu.get_barrier_semaphore()
        pl.semaphore_signal(barrier, 1, device_id=y_nbr, device_id_type=MESH)

        @pl.when(mx == 0)
        def _():
            pl.semaphore_signal(barrier, 1, device_id=x_nbr, device_id_type=MESH)

        for ld in loads[1:]:
            ld.start()
        pl.semaphore_wait(barrier, 1 + mx)

        @pl.when(mx == 1)
        def _():
            pl.semaphore_signal(x_ready, 1, device_id=x_nbr, device_id_type=MESH)

        y_copies = []
        for i in range(n):
            loads[i].wait()
            sbuf[i] = xbuf[i].astype(jnp.bfloat16)
            cp = pltpu.make_async_remote_copy(
                sbuf.at[i], rbuf.at[i], y_send, y_recv.at[i], y_nbr, MESH)
            cp.start()
            y_copies.append(cp)

        @pl.when(mx == 0)
        def _():
            pl.semaphore_wait(x_ready, 1)

        for i, b in enumerate(order):
            y_copies[i].wait_recv()
            total = sbuf[i].astype(jnp.float32) + rbuf[i].astype(jnp.float32)
            o_ref[rows(b), :] = total.astype(o_ref.dtype)
            if i < len(forwarded):
                pltpu.make_async_remote_copy(
                    o_ref.at[rows(b)], o_ref.at[rows(b)], x_send, x_recv, x_nbr, MESH
                ).start()

        x_total = o_ref.at[pl.ds(0, len(forwarded) * ROWS)]
        pltpu.make_async_copy(sbuf, sbuf, y_send).wait()
        pltpu.make_async_copy(x_total, x_total, x_send).wait()
        pltpu.make_async_copy(x_total, x_total, x_recv).wait()

    return pl.pallas_call(
        kernel_body,
        out_shape=jax.ShapeDtypeStruct((M, N), jnp.bfloat16),
        in_specs=[pl.BlockSpec(memory_space=pltpu.HBM)],
        out_specs=pl.BlockSpec(memory_space=pltpu.VMEM),
        scratch_shapes=[
            pltpu.VMEM((n, ROWS, N), jnp.float32),
            pltpu.VMEM((n, ROWS, N), jnp.bfloat16),
            pltpu.VMEM((n, ROWS, N), jnp.bfloat16),
            pltpu.SemaphoreType.DMA((n,)),
            pltpu.SemaphoreType.DMA,
            pltpu.SemaphoreType.DMA((n,)),
            pltpu.SemaphoreType.DMA,
            pltpu.SemaphoreType.DMA,
            pltpu.SemaphoreType.REGULAR,
        ],
        compiler_params=pltpu.CompilerParams(
            collective_id=0,
            disable_bounds_checks=True,
            disable_semaphore_checks=True,
        ),
    )(x)
```

```python
import jax
import jax.numpy as jnp
import numpy as np
from jax import lax
from jax.experimental import pallas as pl
from jax.experimental.pallas import tpu as pltpu

M, N = 1024, 512
HALF = M // 2
MESH = pl.DeviceIdType.MESH

VREG = (8, 128)
ROWS, COLS = 16, 256
PER_ROW = N // COLS
PIECES_PER_HALF = HALF // ROWS * PER_ROW
GROUP = 8


SAMPLE = 4
HEADROOM = 460
ABOVE = 4


def _word(v):
    return np.array(v, np.uint32).view(np.int32)[()]


def _bytes(b):
    return _word(b * 0x01010101)


def _shr(v, k):
    return lax.shift_right_logical(v, jnp.broadcast_to(jnp.int32(k), v.shape))


def _shl(v, k):
    return lax.shift_left(v, jnp.broadcast_to(jnp.int32(k), v.shape))


def _rotl(v, k):
    return _shl(v, k) | _shr(v, 32 - k)


def _at_least(v, n):
    return (v + _bytes(0x80 - n)) & _bytes(0x80)


def _mask(flags):
    return flags - _shr(flags, 7)


def _split(w0, w1):
    q = _rotl(w1, 8)
    swap = (w0 ^ q) & _word(0x7F807F80)
    return w0 ^ swap, _rotl(q ^ swap, 1)


def _join(frac, q):
    swap = (frac ^ q) & _word(0x7F807F80)
    return frac ^ swap, _rotl(q ^ swap, 24)


def _offsets(reference):
    both = reference | _shl(reference, 16)
    each = 255 - _shr(reference, 7)
    each = each | _shl(each, 8)
    return both, each | _shl(each, 16)


def _encode(t, state):
    hi, lo, used, lost = state
    lost = lost | (t & _bytes(0xC0))
    small = _mask(_at_least(t, 8))
    code = t & _bytes(7) & ~small
    n = (((t + _bytes(0x80 - 7)) & small)
         + _shr(_at_least(t, 7 + ABOVE), 7)
         + _shr(_at_least(t, 1) ^ _bytes(0x80), 5))
    end = n + _shl(n, 8)
    end = end + _shl(end, 16)
    lost = lost | (end & _bytes(0xE0))
    end = end & _bytes(0x1F)
    total = _shr(end, 24)
    one = jnp.full(VREG, _word(0x80000000))
    bits = _shl(_shr(one, end & 0xFF) | _shr(one, _shr(end, 8) & 0xFF)
                | _shr(one, _shr(end, 16) & 0xFF) | _shr(one, total), 1)
    at = used & 31
    head, spill = _shr(bits, at), _shl(_shl(bits, 1), 31 - at)
    in_hi = used < 32
    hi = hi | jnp.where(in_hi, head, 0)
    lo = lo | jnp.where(in_hi, spill, head)
    return code, (hi, lo, used + total, lost)


def _decode(code, state):
    hi, lo = state
    escaped = _at_least(code, 1) ^ _bytes(0x80)
    head = hi
    for j in range(4):
        has_suffix = (escaped & _word(0x80 << 8 * j)) != 0
        length = jnp.where(has_suffix, lax.clz(head | 2) + 1, 0)
        head = _shl(head, length)
        n = length if j == 0 else n | _shl(length, 8 * j)
        total = length if j == 0 else total + length
    total = total & 31
    past = _at_least(n, ABOVE + 1)
    small = escaped ^ past ^ _at_least(n, ABOVE)
    t = code | ((n + _bytes(7) - _shr(past, 7)) & _mask(small))
    hi = _shl(hi, total) | _shr(_shr(lo, 1), 31 - total)
    return t, (hi, _shl(lo, total))


def _pack_codes(c):
    return (c[0] | _shl(c[1], 3) | _shl(c[6] & _bytes(3), 6),
            c[2] | _shl(c[3], 3) | _shl(c[7] & _bytes(3), 6),
            c[4] | _shl(c[5], 3) | _shl(c[6] & _bytes(4), 4)
            | _shl(c[7] & _bytes(4), 5))


def _unpack_code(unit, j):
    if j < 6:
        return _shr(unit(j // 2), 3 * (j % 2)) & _bytes(7)
    return ((_shr(unit(j - 6), 6) & _bytes(3))
            | (_shr(unit(2), j - 2) & _bytes(4)))


GROUPS = [list(range(p, p + GROUP)) for p in range(GROUP, PIECES_PER_HALF, GROUP)]
GROUPS += [list(range(GROUP)),
           list(range(PIECES_PER_HALF + 1, PIECES_PER_HALF + GROUP))]
Y_PIECES = [p for group in GROUPS for p in group]
X_PIECES = Y_PIECES[:PIECES_PER_HALF - GROUP + 1]

EARLY = 3
STREAM = []
for _g, _group in enumerate(GROUPS):
    _frac = [("frac", p) for p in _group]
    _code = [("code", _g, k) for k in range(3)]
    if _g == EARLY:
        STREAM += [("suffix", 0), ("suffix", 1)]
    if _g < EARLY:
        STREAM += _frac + _code
    else:
        STREAM += (_code[:1] + _frac[:2] + _code[1:2] + _frac[2:4] + _code[2:]
                   + _frac[4:])
AT = {unit: i for i, unit in enumerate(STREAM)}
Y_UNITS = len(STREAM)
X_UNITS = AT["frac", X_PIECES[-1]] + 1

LOADS = [(8, 1), (9, 1), (10, 2), (12, 4)] + [(p, 8) for p in range(16, 64, 8)]
LOADS += [(0, 8), (64, 4), (68, 4)] + [(p, 14) for p in range(72, 128, 14)]
LOAD_OF = {p + i: j for j, (p, n) in enumerate(LOADS) for i in range(n)}

LATE_ENTRY = 4
UPFRONT = 56
AHEAD = 34
X_LAG = 20
RAW_CHUNKS = 8


def pallas_dist_ar_xy_y_m1024_n512_kernel(
x: jax.Array,
):
    def kernel_body(x_hbm, out, xs, tx, ry, rx, header, raw_tx, raw_rx,
                    load_sems, y_send, y_recv, x_send, x_recv, header_sems,
                    raw_sems, x_entered):
        mx, my = lax.axis_index("x"), lax.axis_index("y")
        y_nbr, x_nbr = (mx, 1 - my), (1 - mx, my)

        def window(p, n=1, shard=False):
            row = p // PER_ROW * ROWS
            if shard:
                half = mx if row < HALF else 1 - mx
                row = pl.multiple_of(half * HALF + row % HALF, ROWS)
            if n == 1:
                return pl.ds(row, ROWS), pl.ds(p % PER_ROW * COLS, COLS)
            return pl.ds(row, n // PER_ROW * ROWS), slice(None)

        loads = [
            pltpu.make_async_copy(x_hbm.at[window(p, n, shard=True)],
                                  xs.at[window(p, n)], load_sems.at[j])
            for j, (p, n) in enumerate(LOADS)
        ]
        loaded = set()

        def local(p):
            if LOAD_OF[p] not in loaded:
                loaded.add(LOAD_OF[p])
                loads[LOAD_OF[p]].wait()
            return xs[window(p)]

        loads[0].start()
        barrier = pltpu.get_barrier_semaphore()
        pl.semaphore_signal(barrier, 1, device_id=y_nbr, device_id_type=MESH)
        loads[1].start()

        @pl.when(mx == 0)
        def _():
            pl.semaphore_signal(barrier, 1, device_id=x_nbr, device_id_type=MESH)

        for load in loads[2:]:
            load.start()

        def meet_peers():
            @pl.when(mx == 0)
            def _():
                pl.semaphore_wait(barrier, 1)

            @pl.when(mx == 1)
            def _():
                pl.semaphore_wait(barrier, 2)
                pl.semaphore_signal(x_entered, 1, device_id=x_nbr,
                                    device_id_type=MESH)

        pl.when(my == 1)(meet_peers)

        y_copies = [
            pltpu.make_async_remote_copy(tx.at[u], ry.at[u], y_send,
                                         y_recv.at[u], y_nbr, MESH)
            for u in range(Y_UNITS)
        ]
        x_copies = [
            pltpu.make_async_remote_copy(ry.at[u], rx.at[u], x_send,
                                         x_recv.at[u], x_nbr, MESH)
            for u in range(X_UNITS)
        ]
        header_y, header_relay, header_x = [
            pltpu.make_async_remote_copy(
                header.at[src], header.at[dst], header_sems.at[2 * k],
                header_sems.at[2 * k + 1], nbr, MESH)
            for k, (src, dst, nbr) in enumerate(
                [(0, 1, y_nbr), (1, 2, x_nbr), (0, 3, x_nbr)])
        ]

        def send(first, stop):
            for u in range(first, stop):
                if STREAM[u] == ("suffix", 0):
                    header_y.start()
                y_copies[u].start()

        def sender():
            state = (jnp.zeros(VREG, jnp.int32),) * 4
            sent, sample = 0, []
            for g, group in enumerate(GROUPS):
                codes = []
                for j, p in enumerate(group):
                    yield True
                    w = pltpu.bitcast(local(p).astype(jnp.bfloat16), jnp.int32)
                    w0, w1 = w[:, :128], w[:, 128:]
                    in_sample = g == 0 and j < SAMPLE
                    if in_sample:
                        flip = _word(0x7FFF7FFF)
                        frac, exp = _split(w0 ^ flip, w1 ^ flip)
                    else:
                        frac, exp = _split(both - w0, both - w1)
                    tx[AT["frac", p]] = frac
                    if g == 0:
                        pl.when(my == 1)(lambda: send(j, j + 1))
                        sent = j + 1
                    pending = [exp]
                    if in_sample:
                        sample.append((w0, w1, exp))
                        if len(sample) < SAMPLE:
                            continue
                        sums = sum((v & 0x7FFF) + (_shr(v, 16) & 0x7FFF)
                                   for s in sample for v in s[:2])
                        mean = (jnp.sum(sums.astype(jnp.float32), keepdims=True)
                                * (1.0 / (SAMPLE * ROWS * COLS)))
                        mean = jnp.broadcast_to(mean, VREG).astype(jnp.int32)
                        reference = jnp.minimum(mean + HEADROOM, 0x7FFF)
                        both, each = _offsets(reference)
                        pending = [s[2] - each for s in sample]
                    for t in pending:
                        code, state = _encode(t, state)
                        codes.append(code)
                codes += [jnp.zeros(VREG, jnp.int32)] * (GROUP - len(codes))
                for k, unit in enumerate(_pack_codes(codes)):
                    tx[AT["code", g, k]] = unit
                if g < EARLY:
                    stop = AT["code", g, 2] + 1
                    pl.when(my == 1)(lambda: send(sent, stop))
                    sent = stop
                if g == LATE_ENTRY:
                    @pl.when(my == 0)
                    def _():
                        meet_peers()
                        send(0, sent)
            hi, lo, used, lost = state
            tx[AT["suffix", 0]] = hi
            tx[AT["suffix", 1]] = lo
            misfit = jnp.where((used > 64) | (lost != 0), 1.0, 0.0)
            misfit = jnp.max(misfit, axis=0, keepdims=True).astype(jnp.int32)
            header[0] = reference[:1] | _shl(misfit, 16)
            yield True
            header_x.start()

        def receiver(buf, slot, pieces, shift):
            yield AT["suffix", 1]
            if slot == 2:
                header_relay.wait_recv()
            both, each = _offsets(jnp.broadcast_to(header[slot], VREG) & 0x7FFF)
            state = buf[AT["suffix", 0]], buf[AT["suffix", 1]]
            for i, p in enumerate(pieces):
                g, j = divmod(i, GROUP)
                yield AT["code", g, min(j // 2, 2)]
                code = _unpack_code(lambda k: buf[AT["code", g, k]], j)
                t, state = _decode(code, state)
                q = _rotl(t + each if i < SAMPLE else t, 31)
                yield AT["frac", p]
                words = _join(buf[AT["frac", p]], q)
                if i < SAMPLE:
                    words = [v ^ _word(0x7FFF7FFF) for v in words]
                else:
                    words = [both - v for v in words]
                other = pltpu.bitcast(jnp.concatenate(words, axis=1), jnp.bfloat16)
                total = local(p + shift) + other.astype(jnp.float32)
                out[window(p + shift, shard=True)] = total.astype(out.dtype)

        encoding = sender()
        for _ in range(UPFRONT + 1):
            next(encoding)

        @pl.when(mx == 0)
        def _():
            pl.semaphore_wait(x_entered, 1)

        from_y = receiver(ry, 1, Y_PIECES, 0)
        from_x = receiver(rx, 2, X_PIECES, PIECES_PER_HALF)
        y_next, x_next = next(from_y), next(from_x)
        sent = AT["suffix", 0]
        steps = max(Y_UNITS, X_UNITS + X_LAG)
        for u in range(steps):
            if u == steps - 6:
                header_x.wait_recv()
                for copy in (header_y, header_relay, header_x):
                    copy.wait_send()
                flags = header[0] | header[1] | header[2] | header[3]
                misfit = jnp.max(_shr(flags, 16).astype(jnp.float32)) > 0
            if u == steps - 2:
                pltpu.make_async_copy(tx, tx, y_send).wait()
                pltpu.make_async_copy(rx, rx, x_send).wait()
            if u < Y_UNITS:
                if STREAM[u] == ("suffix", 0):
                    header_y.wait_recv()
                    header_relay.start()
                y_copies[u].wait_recv()
            if u < X_UNITS:
                x_copies[u].start()
            for _ in range(3 if u >= 2 else 0):
                if encoding and not next(encoding, False):
                    encoding = None
            if not encoding:
                stop = min(u + AHEAD, Y_UNITS)
                send(sent, stop)
                sent = stop
            if 0 <= u - X_LAG < X_UNITS:
                x_copies[u - X_LAG].wait_recv()
            for _ in range(4):
                if y_next is not None and y_next <= u:
                    y_next = next(from_y, None)
                if x_next is not None and x_next <= u - X_LAG:
                    x_next = next(from_x, None)
        assert y_next is None and x_next is None and len(loaded) == len(LOADS)

        @pl.when(misfit)
        def _plain_bfloat16_exchange():
            rows = HALF // RAW_CHUNKS

            def own(i):
                return xs[pl.ds(pl.multiple_of(i * rows, rows), rows)]

            def y_copy(i):
                return pltpu.make_async_remote_copy(
                    raw_tx.at[i], raw_rx.at[i], raw_sems.at[0],
                    raw_sems.at[3 + i], y_nbr, MESH)

            @pl.loop(0, RAW_CHUNKS)
            def _(i):
                raw_tx[i] = own(i).astype(jnp.bfloat16)
                y_copy(i).start()

            @pl.loop(0, RAW_CHUNKS)
            def _(i):
                y_copy(i).wait_recv()
                pltpu.make_async_remote_copy(
                    raw_rx.at[i], raw_rx.at[RAW_CHUNKS + i], raw_sems.at[1],
                    raw_sems.at[2], x_nbr, MESH).start()

            for k in range(3):
                pltpu.make_async_copy(raw_tx, raw_tx, raw_sems.at[k]).wait()

            @pl.loop(0, 2 * RAW_CHUNKS)
            def _(i):
                row = pl.multiple_of((mx * HALF + i * rows) % M, rows)
                total = own(i) + raw_rx[i].astype(jnp.float32)
                out[pl.ds(row, rows)] = total.astype(out.dtype)

    raw_chunk = (HALF // RAW_CHUNKS, N)
    return pl.pallas_call(
        kernel_body,
        out_shape=jax.ShapeDtypeStruct((M, N), jnp.bfloat16),
        in_specs=[pl.BlockSpec(memory_space=pltpu.HBM)],
        out_specs=pl.BlockSpec(memory_space=pltpu.VMEM),
        scratch_shapes=[
            pltpu.VMEM((M, N), jnp.float32),
            pltpu.VMEM((Y_UNITS, *VREG), jnp.int32),
            pltpu.VMEM((Y_UNITS, *VREG), jnp.int32),
            pltpu.VMEM((X_UNITS, *VREG), jnp.int32),
            pltpu.VMEM((4, 1, 128), jnp.int32),
            pltpu.VMEM((RAW_CHUNKS, *raw_chunk), jnp.bfloat16),
            pltpu.VMEM((2 * RAW_CHUNKS, *raw_chunk), jnp.bfloat16),
            pltpu.SemaphoreType.DMA((len(LOADS),)),
            pltpu.SemaphoreType.DMA,
            pltpu.SemaphoreType.DMA((Y_UNITS,)),
            pltpu.SemaphoreType.DMA,
            pltpu.SemaphoreType.DMA((X_UNITS,)),
            pltpu.SemaphoreType.DMA((6,)),
            pltpu.SemaphoreType.DMA((3 + RAW_CHUNKS,)),
            pltpu.SemaphoreType.REGULAR,
        ],
        compiler_params=pltpu.CompilerParams(
            collective_id=0,
            disable_bounds_checks=True,
            disable_semaphore_checks=True,
        ),
    )(x)
```

```python
import jax
import jax.numpy as jnp
import numpy as np
from jax import lax
from jax.experimental import pallas as pl
from jax.experimental.pallas import tpu as pltpu

M, N = 1024, 512
HALF = M // 2
MESH = pl.DeviceIdType.MESH

VREG = (8, 128)
ROWS, COLS = 16, 256
PER_ROW = N // COLS
PIECES_PER_HALF = HALF // ROWS * PER_ROW
GROUP = 4


SAMPLE = GROUP
HEADROOM = 532
NEAR, FAR = 4, 18
WORDS = 10
OWN = 6
POOL_BITS = 176


def _word(v):
    return np.array(v, np.uint32).view(np.int32)[()]


def _bytes(b):
    return _word(b * 0x01010101)


def _shr(v, k):
    if isinstance(k, int):
        return lax.shift_right_logical(v, np.int32(k)) if k else v
    return lax.shift_right_logical(v, k)


def _shl(v, k):
    if isinstance(k, int):
        return lax.shift_left(v, np.int32(k)) if k else v
    return lax.shift_left(v, k)


def _rotl(v, k):
    return _shl(v, k) | _shr(v, 32 - k)


def _window(first, second, k):
    return _shl(first, k) | _shr(_shr(second, 1), 31 - k)


def _at_least(v, n):
    return (v + _bytes(0x80 - n)) & _bytes(0x80)


def _mask(flags):
    return flags - _shr(flags, 7)


def _split(w0, w1):
    q = _rotl(w1, 8)
    swap = (w0 ^ q) & _word(0x7F807F80)
    return w0 ^ swap, _rotl(q ^ swap, 1)


def _join(frac, q):
    swap = (frac ^ q) & _word(0x7F807F80)
    return frac ^ swap, _rotl(q ^ swap, 24)


def _offsets(reference):
    both = reference | _shl(reference, 16)
    each = 255 - _shr(reference, 7)
    each = each | _shl(each, 8)
    return both, each | _shl(each, 16)


def _encode(t, state):
    words, last, used, lost = state
    lost = lost | (t & _bytes(0xC0))
    small = _mask(_at_least(t, 5))
    ge1, ge2 = _at_least(t, 1), _at_least(t, 2)
    code = (t + _bytes(3)) & _bytes(3) & ~small & _mask(ge2)
    is0, is1 = ge1 ^ _bytes(0x80), ge1 ^ ge2
    n = (((t + _bytes(0x80 - 4)) & small)
         + _shr(_at_least(t, 4 + NEAR), 7) + _shr(_at_least(t, 3 + FAR), 7)
         + (_shr(is1, 5) | _shr(is0, 3) | _shr(is0, 6)))
    end = n + (_shl(n, 8) & _word(0xFF00FF00))
    lost = lost | (end & _bytes(0xE0))
    end = end & _bytes(0x1F)
    one = jnp.full(VREG, _word(0x80000000))
    for half in (end & 0xFFFF, _shr(end, 16)):
        total = _shr(half, 8)
        bits = _shl(_shr(one, half & 0xFF) | _shr(one, total), 1)
        at, index = used & 31, _shr(used, 5)
        last = last | _shr(bits, at)
        words = [lax.select(index == i, last, w) for i, w in enumerate(words)]
        last = lax.select(at + total >= 32, _shl(_shl(bits, 1), 31 - at), last)
        used = used + total
    return code, (words, last, used, lost)


def _decode(code, state):
    words, at = state
    escaped = _at_least(code, 1) ^ _bytes(0x80)
    masks = _shr(escaped, 2) - _shr(escaped, 7)
    for pair in ((0, 1), (2, 3)):
        head = _window(words[0], words[1], at)
        for j in pair:
            mask = _shr(masks, 8 * j) & 31
            one, run = mask & 1, lax.clz(head) & mask
            head = _shl(_shl(head, one), run)
            at = at + one + run
            zeros = run if j == 0 else zeros | _shl(run, 8 * j)
        full = at >= 32
        words = [lax.select(full, b, a)
                 for a, b in zip(words, words[1:])] + words[-1:]
        at = at & 31
    near, far = _at_least(zeros, NEAR), _at_least(zeros, FAR)
    is1 = near ^ _at_least(zeros, NEAR - 1)
    is0 = far ^ _at_least(zeros, FAR - 1)
    small = _mask(escaped ^ is1 ^ is0)
    t = (((code + _bytes(1)) & ~_mask(escaped)) | _shr(is1, 7)
         | ((zeros + _bytes(5) - _shr(near, 7) - _shr(far, 7)) & small))
    return t, (words, at)


def _close(state, reference):
    words, last, used, lost = state
    index = _shr(used, 5)
    words = [lax.select(index == i, last, w) for i, w in enumerate(words)]
    row = lax.broadcasted_iota(jnp.int32, VREG, 0)
    excess = jnp.maximum(used - 32 * OWN, 0)
    end = excess
    for k in (1, 2, 4):
        end = end + jnp.where(row >= k, pltpu.roll(end, k, 0), 0)
    misfit = (lost != 0) | (used > 32 * WORDS) | (end > POOL_BITS)
    start = (end - excess) & 0xFF
    at, index = start & 31, _shr(start, 5)
    zero = jnp.zeros(VREG, jnp.int32)
    tail = words[OWN:]
    moved = [_shr(b, at) | _shl(_shl(a, 1), 31 - at)
             for a, b in zip([zero] + tail, tail + [zero])]
    rows = [zero] * 8
    for i in range(6):
        for j, w in enumerate(moved[:i + 1]):
            rows[i] = lax.select(index == i - j, w, rows[i])
    rows[5] = ((rows[5] & _word(0xFFFF0000)) | reference
               | jnp.where(misfit, 0x8000, 0))
    start = _shl(start, 8 * (row & 3))
    rows[6], rows[7] = jnp.where(row < 4, start, 0), jnp.where(row < 4, 0, start)
    unit = zero
    for i, w in enumerate(rows):
        for k in (1, 2, 4):
            w = w | pltpu.roll(w, k, 0)
        unit = lax.select(row == i, w, unit)
    return words[:OWN] + [unit]


def _reopen(own, pool_row):
    rows = [jnp.broadcast_to(pool_row(i), VREG) for i in range(8)]
    row = lax.broadcasted_iota(jnp.int32, VREG, 0)
    start = _shr(lax.select(row < 4, rows[6], rows[7]), 8 * (row & 3)) & 0xFF
    at, index = start & 31, _shr(start, 5)
    moved = []
    for j in range(WORDS - OWN + 1):
        w = rows[5]
        for i in range(j, 5):
            w = lax.select(index == i - j, rows[i], w)
        moved.append(w)
    tail = [_window(a, b, at) for a, b in zip(moved, moved[1:])]
    return (own + tail, jnp.zeros(VREG, jnp.int32)), rows[5] & 0x7FFF


EXTRA = 8
X_PIECES = list(range(EXTRA, PIECES_PER_HALF))
Y_PIECES = (X_PIECES + list(range(EXTRA))
            + list(range(PIECES_PER_HALF, PIECES_PER_HALF + EXTRA)))

EARLY = 6
STREAM = []
for _g in range(len(Y_PIECES) // GROUP):
    _frac = [("frac", i) for i in range(_g * GROUP, (_g + 1) * GROUP)]
    if _g == EARLY:
        STREAM += [("suffix", k) for k in range(OWN + 1)]
    STREAM += _frac + [("code", _g)] if _g < EARLY else [("code", _g)] + _frac
AT = {unit: i for i, unit in enumerate(STREAM)}
Y_UNITS = len(STREAM)
X_UNITS = AT["frac", len(X_PIECES) - 1] + 1
POOL = AT["suffix", OWN]

LOADS = [(8, 1), (9, 1), (10, 2), (12, 4)] + [(p, 8) for p in range(16, 64, 8)]
LOADS += [(0, 8), (64, 8)] + [(p, 28) for p in (72, 100)]
LOAD_OF = {p + i: j for j, (p, n) in enumerate(LOADS) for i in range(n)}

LATE_ENTRY = 7
UPFRONT = 48
AHEAD = 40
X_LAG = 20
RAW_CHUNKS = 8


def pallas_dist_ar_xy_y_m1024_n512_kernel(
x: jax.Array,
):
    def kernel_body(x_hbm, out, xs, tx, ry, rx, x_status, raw_tx, raw_rx,
                    load_sems, y_send, y_recv, x_send, x_recv, status_sems,
                    raw_sems, x_entered):
        mx, my = lax.axis_index("x"), lax.axis_index("y")
        y_nbr, x_nbr = (mx, 1 - my), (1 - mx, my)

        def window(p, n=1, shard=False):
            row = p // PER_ROW * ROWS
            if shard:
                half = mx if row < HALF else 1 - mx
                row = pl.multiple_of(half * HALF + row % HALF, ROWS)
            if n == 1:
                return pl.ds(row, ROWS), pl.ds(p % PER_ROW * COLS, COLS)
            return pl.ds(row, n // PER_ROW * ROWS), slice(None)

        loads = [
            pltpu.make_async_copy(x_hbm.at[window(p, n, shard=True)],
                                  xs.at[window(p, n)], load_sems.at[j])
            for j, (p, n) in enumerate(LOADS)
        ]
        loaded = set()

        def local(p):
            if LOAD_OF[p] not in loaded:
                loaded.add(LOAD_OF[p])
                loads[LOAD_OF[p]].wait()
            return xs[window(p)]

        loads[0].start()
        barrier = pltpu.get_barrier_semaphore()
        pl.semaphore_signal(barrier, 1, device_id=y_nbr, device_id_type=MESH)
        loads[1].start()

        @pl.when(mx == 0)
        def _():
            pl.semaphore_signal(barrier, 1, device_id=x_nbr, device_id_type=MESH)

        for load in loads[2:]:
            load.start()

        def meet_peers():
            @pl.when(mx == 0)
            def _():
                pl.semaphore_wait(barrier, 1)

            @pl.when(mx == 1)
            def _():
                pl.semaphore_wait(barrier, 2)
                pl.semaphore_signal(x_entered, 1, device_id=x_nbr,
                                    device_id_type=MESH)

        pl.when(my == 1)(meet_peers)

        y_copies = [
            pltpu.make_async_remote_copy(tx.at[u], ry.at[u], y_send,
                                         y_recv.at[u], y_nbr, MESH)
            for u in range(Y_UNITS)
        ]
        x_copies = [
            pltpu.make_async_remote_copy(ry.at[u], rx.at[u], x_send,
                                         x_recv.at[u], x_nbr, MESH)
            for u in range(X_UNITS)
        ]
        status_row = pl.ds(5, 1)
        status = pltpu.make_async_remote_copy(
            tx.at[POOL, status_row], x_status.at[status_row], status_sems.at[0],
            status_sems.at[1], x_nbr, MESH)

        def send(first, stop):
            for u in range(first, stop):
                y_copies[u].start()

        def sender():
            zero = jnp.zeros(VREG, jnp.int32)
            state = [zero] * WORDS, zero, zero, zero
            sent, sample = 0, []
            for i, p in enumerate(Y_PIECES):
                yield True
                w = pltpu.bitcast(local(p).astype(jnp.bfloat16), jnp.int32)
                w0, w1 = w[:, :128], w[:, 128:]
                if i < SAMPLE:
                    flip = _word(0x7FFF7FFF)
                    frac, exp = _split(w0 ^ flip, w1 ^ flip)
                    tx[AT["frac", i]] = frac
                    pl.when(my == 1)(lambda: send(i, i + 1))
                    sent = i + 1
                    sample.append((w0, w1, exp))
                    if len(sample) < SAMPLE:
                        continue
                    sums = sum((v & 0x7FFF) + (_shr(v, 16) & 0x7FFF)
                               for s in sample for v in s[:2])
                    mean = (jnp.sum(sums.astype(jnp.float32), keepdims=True)
                            * (1.0 / (SAMPLE * ROWS * COLS)))
                    mean = jnp.broadcast_to(mean, VREG).astype(jnp.int32)
                    reference = jnp.minimum(mean + HEADROOM, 0x7FFF)
                    both, each = _offsets(reference)
                    pending = list(enumerate(s[2] - each for s in sample))
                else:
                    frac, exp = _split(both - w0, both - w1)
                    tx[AT["frac", i]] = frac
                    pending = [(i % GROUP, exp)]
                for j, t in pending:
                    code, state = _encode(t, state)
                    codes = code if j == 0 else codes | _shl(code, 2 * j)
                g = i // GROUP
                if i % GROUP < GROUP - 1:
                    continue
                tx[AT["code", g]] = codes
                if g < EARLY:
                    stop = AT["code", g] + 1
                    pl.when(my == 1)(lambda: send(sent, stop))
                    sent = stop
                if g == LATE_ENTRY:
                    @pl.when(my == 0)
                    def _():
                        meet_peers()
                        send(0, sent)
            yield True
            yield True
            for k, unit in enumerate(_close(state, reference)):
                tx[AT["suffix", k]] = unit
            status.start()

        def receiver(buf, pieces, shift):
            yield POOL
            state, reference = _reopen(
                [buf[AT["suffix", k]] for k in range(OWN)],
                lambda i: buf[POOL, pl.ds(i, 1)])
            both, each = _offsets(reference)
            for i, p in enumerate(pieces):
                g, j = divmod(i, GROUP)
                yield AT["code", g]
                code = _shr(buf[AT["code", g]], 2 * j) & _bytes(3)
                t, state = _decode(code, state)
                q = _rotl(t + each if i < SAMPLE else t, 31)
                yield AT["frac", i]
                words = _join(buf[AT["frac", i]], q)
                if i < SAMPLE:
                    words = [v ^ _word(0x7FFF7FFF) for v in words]
                else:
                    words = [both - v for v in words]
                other = pltpu.bitcast(jnp.concatenate(words, axis=1), jnp.bfloat16)
                total = local(p + shift) + other.astype(jnp.float32)
                out[window(p + shift, shard=True)] = total.astype(out.dtype)

        encoding = sender()
        for _ in range(UPFRONT + 1):
            next(encoding)

        @pl.when(mx == 0)
        def _():
            pl.semaphore_wait(x_entered, 1)

        from_y = receiver(ry, Y_PIECES, 0)
        from_x = receiver(rx, X_PIECES, PIECES_PER_HALF)
        y_next, x_next = next(from_y), next(from_x)
        sent = AT["suffix", 0]
        steps = max(Y_UNITS, X_UNITS + X_LAG)
        for u in range(steps):
            if u == steps - 6:
                status.wait()
                flags = (tx[POOL, status_row] | ry[POOL, status_row]
                         | rx[POOL, status_row] | x_status[status_row])
                misfit = jnp.max((flags & 0x8000).astype(jnp.float32)) > 0
            if u == steps - 2:
                pltpu.make_async_copy(tx, tx, y_send).wait()
                pltpu.make_async_copy(rx, rx, x_send).wait()
            if u < Y_UNITS:
                y_copies[u].wait_recv()
            if u < X_UNITS:
                x_copies[u].start()
            if 0 <= u - X_LAG < X_UNITS:
                x_copies[u - X_LAG].wait_recv()
            for _ in range(3):
                if encoding and not next(encoding, False):
                    encoding = None
            if not encoding:
                stop = min(sent + 4, u + AHEAD, Y_UNITS)
                send(sent, stop)
                sent = stop
            for k in range(4):
                if y_next is not None and y_next <= u:
                    y_next = next(from_y, None)
                if k < 3 and x_next is not None and x_next <= u - X_LAG:
                    x_next = next(from_x, None)
        assert y_next is None and x_next is None and len(loaded) == len(LOADS)

        @pl.when(misfit)
        def _plain_bfloat16_exchange():
            rows = HALF // RAW_CHUNKS

            def own(i):
                return xs[pl.ds(pl.multiple_of(i * rows, rows), rows)]

            def y_copy(i):
                return pltpu.make_async_remote_copy(
                    raw_tx.at[i], raw_rx.at[i], raw_sems.at[0],
                    raw_sems.at[3 + i], y_nbr, MESH)

            @pl.loop(0, RAW_CHUNKS)
            def _(i):
                raw_tx[i] = own(i).astype(jnp.bfloat16)
                y_copy(i).start()

            @pl.loop(0, RAW_CHUNKS)
            def _(i):
                y_copy(i).wait_recv()
                pltpu.make_async_remote_copy(
                    raw_rx.at[i], raw_rx.at[RAW_CHUNKS + i], raw_sems.at[1],
                    raw_sems.at[2], x_nbr, MESH).start()

            for k in range(3):
                pltpu.make_async_copy(raw_tx, raw_tx, raw_sems.at[k]).wait()

            @pl.loop(0, 2 * RAW_CHUNKS)
            def _(i):
                row = pl.multiple_of((mx * HALF + i * rows) % M, rows)
                total = own(i) + raw_rx[i].astype(jnp.float32)
                out[pl.ds(row, rows)] = total.astype(out.dtype)

    raw_chunk = (HALF // RAW_CHUNKS, N)
    return pl.pallas_call(
        kernel_body,
        out_shape=jax.ShapeDtypeStruct((M, N), jnp.bfloat16),
        in_specs=[pl.BlockSpec(memory_space=pltpu.HBM)],
        out_specs=pl.BlockSpec(memory_space=pltpu.VMEM),
        scratch_shapes=[
            pltpu.VMEM((M, N), jnp.float32),
            pltpu.VMEM((Y_UNITS, *VREG), jnp.int32),
            pltpu.VMEM((Y_UNITS, *VREG), jnp.int32),
            pltpu.VMEM((X_UNITS, *VREG), jnp.int32),
            pltpu.VMEM(VREG, jnp.int32),
            pltpu.VMEM((RAW_CHUNKS, *raw_chunk), jnp.bfloat16),
            pltpu.VMEM((2 * RAW_CHUNKS, *raw_chunk), jnp.bfloat16),
            pltpu.SemaphoreType.DMA((len(LOADS),)),
            pltpu.SemaphoreType.DMA,
            pltpu.SemaphoreType.DMA((Y_UNITS,)),
            pltpu.SemaphoreType.DMA,
            pltpu.SemaphoreType.DMA((X_UNITS,)),
            pltpu.SemaphoreType.DMA((2,)),
            pltpu.SemaphoreType.DMA((3 + RAW_CHUNKS,)),
            pltpu.SemaphoreType.REGULAR,
        ],
        compiler_params=pltpu.CompilerParams(
            collective_id=0,
            disable_bounds_checks=True,
            disable_semaphore_checks=True,
        ),
    )(x)
```

```python
import functools

import jax
import jax.numpy as jnp
import numpy as np
from jax import lax
from jax.experimental import pallas as pl
from jax.experimental.pallas import tpu as pltpu

M, N = 1024, 512
MESH = pl.DeviceIdType.MESH

VREG = (8, 128)
PIECE = (16, 256)
BLOCK = 32


HEADROOM = 532
NEAR, FAR = 4, 18
WORDS = 10
OWN = 6
POOL_BITS = 176
HEADER_ROW = 5
MISFIT = 0x8000


def _word(v):
    return np.array(v, np.uint32).view(np.int32)[()]


def _bytes(b):
    return _word(b * 0x01010101)


def _shr(v, k):
    if isinstance(k, int):
        return lax.shift_right_logical(v, np.int32(k)) if k else v
    return lax.shift_right_logical(v, k)


def _shl(v, k):
    if isinstance(k, int):
        return lax.shift_left(v, np.int32(k)) if k else v
    return lax.shift_left(v, k)


def _rotl(v, k):
    return _shl(v, k) | _shr(v, 32 - k)


def _window(first, second, k):
    return _shl(first, k) | _shr(_shr(second, 1), 31 - k)


def _at_least(v, n):
    return (v + _bytes(0x80 - n)) & _bytes(0x80)


def _mask(flags):
    return flags - _shr(flags, 7)


def _split(w0, w1):
    q = _rotl(w1, 8)
    swap = (w0 ^ q) & _word(0x7F807F80)
    return w0 ^ swap, _rotl(q ^ swap, 1)


def _join(frac, q):
    swap = (frac ^ q) & _word(0x7F807F80)
    return frac ^ swap, _rotl(q ^ swap, 24)


def _offsets(reference):
    both = reference | _shl(reference, 16)
    each = 255 - _shr(reference, 7)
    each = each | _shl(each, 8)
    return both, each | _shl(each, 16)


def _encode(t, state):
    words, last, used, lost = state
    lost = lost | (t & _bytes(0xC0))
    ge1, ge2, ge5 = _at_least(t, 1), _at_least(t, 2), _at_least(t, 5)
    code = (t + _bytes(3)) & _bytes(3) & _mask(ge2 ^ ge5)
    is0, is1 = ge1 ^ _bytes(0x80), ge1 ^ ge2
    n = (((t + _bytes(0x80 - 4)) & _mask(ge5))
         + _shr(_at_least(t, 4 + NEAR), 7) + _shr(_at_least(t, 3 + FAR), 7)
         + (_shr(is1, 5) | _shr(is0, 3) | _shr(is0, 6)))
    end = n + (_shl(n, 8) & _word(0xFF00FF00))
    lost = lost | (end & _bytes(0xE0))
    end = end & _bytes(0x1F)
    one = jnp.full(VREG, _word(0x80000000))
    for pair in (end & 0xFFFF, _shr(end, 16)):
        total = _shr(pair, 8)
        bits = _shl(_shr(one, pair & 0xFF) | _shr(one, total), 1)
        at = used & 31
        last = last | _shr(bits, at)
        full = at + total >= 32
        words = [lax.select(full, b, a) for a, b in zip(words, words[1:] + [last])]
        last = lax.select(full, _shl(_shl(bits, 1), 31 - at), last)
        used = used + total
    return code, (words, last, used, lost)


def _decode(code, state):
    words, at = state
    escaped = (_bytes(0x80) - code) & _bytes(0x80)
    ones = _shr(escaped, 7)
    masks = _shr(escaped, 2) - ones
    for pair in ((0, 1), (2, 3)):
        head = _window(words[0], words[1], at)
        for j in pair:
            mask = _shr(masks, 8 * j) & 31 if j < 3 else _shr(masks, 24)
            one, run = mask & 1, lax.clz(head) & mask
            head = _shl(_shl(head, one), run)
            at = at + one + run
            zeros = run if j == 0 else zeros | _shl(run, 8 * j)
        full = at >= 32
        words = [lax.select(full, b, a)
                 for a, b in zip(words, words[1:])] + words[-1:]
        at = at & 31
    near, far = _at_least(zeros, NEAR), _at_least(zeros, FAR)
    is1 = near ^ _at_least(zeros, NEAR - 1)
    is0 = far ^ _at_least(zeros, FAR - 1)
    t = ((code + _bytes(1) - ones) | _shr(is1, 7)
         | ((zeros + _bytes(5) - _shr(near, 7) - _shr(far, 7))
            & _mask(escaped ^ is1 ^ is0)))
    return t, (words, at)


def _close(state, reference):
    words, last, used, lost = state
    zero = jnp.zeros(VREG, jnp.int32)
    words, unused = words + [last], WORDS - _shr(used, 5)
    for k in (1, 2, 4, 8):
        words = [lax.select((unused & k) != 0, b, a)
                 for a, b in zip(words, words[k:] + [zero] * k)]
    row = lax.broadcasted_iota(jnp.int32, VREG, 0)
    excess = jnp.maximum(used - 32 * OWN, 0)
    end = excess
    for k in (1, 2, 4):
        end = end + jnp.where(row >= k, pltpu.roll(end, k, 0), 0)
    misfit = (lost != 0) | (used > 32 * WORDS) | (end > POOL_BITS)
    start = (end - excess) & 0xFF
    at, index = start & 31, _shr(start, 5)
    tail = words[OWN:WORDS]
    moved = [_shr(b, at) | _shl(_shl(a, 1), 31 - at)
             for a, b in zip([zero] + tail, tail + [zero])]
    rows = [zero] * 8
    for i in range(6):
        for j, w in enumerate(moved[:i + 1]):
            rows[i] = lax.select(index == i - j, w, rows[i])
    rows[HEADER_ROW] = ((rows[HEADER_ROW] & _word(0xFFFF0000)) | reference
                        | jnp.where(misfit, MISFIT, 0))
    start = _shl(start, 8 * (row & 3))
    rows[6], rows[7] = jnp.where(row < 4, start, 0), jnp.where(row < 4, 0, start)
    unit = zero
    for i, w in enumerate(rows):
        for k in (1, 2, 4):
            w = w | pltpu.roll(w, k, 0)
        unit = lax.select(row == i, w, unit)
    return words[:OWN] + [unit]


def _reopen(own, pool_row):
    rows = [jnp.broadcast_to(pool_row(i), VREG) for i in range(8)]
    row = lax.broadcasted_iota(jnp.int32, VREG, 0)
    start = _shr(lax.select(row < 4, rows[6], rows[7]), 8 * (row & 3)) & 0xFF
    at, index = start & 31, _shr(start, 5)
    moved = []
    for j in range(WORDS - OWN + 1):
        w = rows[5]
        for i in range(j, 5):
            w = lax.select(index == i - j, rows[i], w)
        moved.append(w)
    tail = [_window(a, b, at) for a, b in zip(moved, moved[1:])]
    return (own + tail, jnp.zeros(VREG, jnp.int32)), rows[HEADER_ROW] & 0x7FFF


BLOCKS = M // BLOCK
Y_BLOCKS = 18
X_BLOCKS = BLOCKS - Y_BLOCKS
Y_UNITS = 5 * Y_BLOCKS + OWN + 1
X_UNITS = 5 * X_BLOCKS + OWN + 1
X_LAG = 5 * (Y_BLOCKS - X_BLOCKS)

EARLY = 6
SUFFIX = 5 * EARLY
POOL = SUFFIX + OWN
UPFRONT = (12, 15)

ROUNDS = X_BLOCKS // 2
BACKLOG = Y_BLOCKS - ROUNDS
ROUNDS_START = 5 * BACKLOG + OWN + 1
BACKLOG_START = ROUNDS_START - 2 * BACKLOG - BACKLOG // 3
PACED = Y_UNITS - 2 * (BACKLOG_START - 2 * (Y_BLOCKS - min(UPFRONT) + 1))
assert PACED > SUFFIX and BACKLOG_START > POOL

RAW_CHUNKS = 8
RAW_ROWS = M // 2 // RAW_CHUNKS


def _where(cond, a, b):
    return (a if cond else b) if isinstance(cond, bool) else jnp.where(cond, a, b)


def _frac_at(g, j):
    return 5 * g + j + _where(g < EARLY, 0, OWN + 2)


def _code_at(g):
    return 5 * g + _where(g < EARLY, 4, OWN + 1)


def pallas_dist_ar_xy_y_m1024_n512_kernel(
x: jax.Array,
):
    def kernel_body(x_hbm, out, xs, tx, ry, rx, x_header, raw_tx, raw_rx,
                    load_sems, y_send, y_recv, x_send, x_recv, header_sems,
                    raw_sems, x_entered):
        mx, my = lax.axis_index("x"), lax.axis_index("y")
        y_nbr, x_nbr = (mx, 1 - my), (1 - mx, my)

        def first_row(g, sender_mx):
            return pl.multiple_of((g ^ sender_mx * (BLOCKS - 1)) * BLOCK, BLOCK)

        def piece(g, j, sender_mx):
            row = first_row(g, sender_mx) + j // 2 * PIECE[0]
            return (pl.ds(pl.multiple_of(row, PIECE[0]), PIECE[0]),
                    pl.ds(j % 2 * PIECE[1], PIECE[1]))

        def load(window, sem):
            return pltpu.make_async_copy(x_hbm.at[window], xs.at[window], sem)

        def load_piece(j):
            return load(piece(0, j, mx), load_sems.at[Y_BLOCKS + j])

        def load_block(g):
            return load(pl.ds(first_row(g, mx), BLOCK), load_sems.at[g])

        def y_copy(u):
            return pltpu.make_async_remote_copy(
                tx.at[u], ry.at[u], y_send, y_recv.at[u], y_nbr, MESH)

        landed = rx.at[pl.ds(0, ROUNDS_START - X_LAG)]

        def x_copy(u):
            sem = x_recv.at[jnp.maximum(u - (ROUNDS_START - X_LAG) + 1, 0)]
            return pltpu.make_async_remote_copy(
                ry.at[u], rx.at[u], x_send, sem, x_nbr, MESH)

        def relay(u):
            y_copy(u).wait_recv()
            x_copy(u).start()

        load_piece(0).start()
        barrier = pltpu.get_barrier_semaphore()
        pl.semaphore_signal(barrier, 1, device_id=y_nbr, device_id_type=MESH)
        for j in range(1, 4):
            load_piece(j).start()

        @pl.when(mx == 0)
        def _():
            pl.semaphore_signal(barrier, 1, device_id=x_nbr, device_id_type=MESH)

        for g in range(1, Y_BLOCKS):
            load_block(g).start()
        rest = pl.multiple_of((1 - mx) * Y_BLOCKS * BLOCK, BLOCK)
        load_rest = load(pl.ds(rest, X_BLOCKS * BLOCK), load_sems.at[0])
        load_rest.start()

        def meet_peers():
            @pl.when(mx == 0)
            def _():
                pl.semaphore_wait(barrier, 1)

            @pl.when(mx == 1)
            def _():
                pl.semaphore_wait(barrier, 2)
                pl.semaphore_signal(x_entered, 1, device_id=x_nbr,
                                    device_id_type=MESH)

        pl.when(my == 1)(meet_peers)

        def words_of(g, j):
            w = pltpu.bitcast(xs[piece(g, j, mx)].astype(jnp.bfloat16), jnp.int32)
            return w[:, :128], w[:, 128:]

        flip = _word(0x7FFF7FFF)
        sums, exps = 0, []
        for j in range(4):
            load_piece(j).wait()
            w0, w1 = words_of(0, j)
            tx[j], exp = _split(w0 ^ flip, w1 ^ flip)
            pl.when(my == 1)(lambda: y_copy(j).start())
            exps.append(exp)
            for w in (w0, w1):
                sums = sums + (w & 0x7FFF) + (_shr(w, 16) & 0x7FFF)
        mean = jnp.sum(sums.astype(jnp.float32), keepdims=True) * (1 / (BLOCK * N))
        mean = jnp.broadcast_to(mean, VREG).astype(jnp.int32)
        reference = jnp.minimum(mean + HEADROOM, 0x7FFF)
        both, each = _offsets(reference)
        zero = jnp.zeros(VREG, jnp.int32)
        state, codes = ([zero] * WORDS, zero, zero, zero), zero
        for j, exp in enumerate(exps):
            code, state = _encode(exp - each, state)
            codes = codes | _shl(code, 2 * j)
        tx[4] = codes
        pl.when(my == 1)(lambda: y_copy(4).start())

        def encode_block(g, state, halfway=lambda: None):
            load_block(g).wait()
            codes = zero
            for j in range(4):
                if j == 2:
                    halfway()
                w0, w1 = words_of(g, j)
                tx[_frac_at(g, j)], exp = _split(both - w0, both - w1)
                code, state = _encode(exp, state)
                codes = codes | _shl(code, 2 * j)
            tx[_code_at(g)] = codes
            return state

        def encode_and_send(g, state):
            state = encode_block(g, state)

            @pl.when((my == 1) & (g < EARLY))
            def _():
                for k in range(5):
                    y_copy(5 * g + k).start()

            @pl.when((my == 0) & (g == EARLY - 1))
            def _():
                meet_peers()
                for u in range(SUFFIX):
                    y_copy(u).start()

            return state

        def encode_and_relay(g, state):
            u = 2 * (g - upfront)
            relay(u)
            return encode_block(g, state, lambda: relay(u + 1))

        upfront = jnp.where(my == 0, *UPFRONT)
        state = lax.fori_loop(1, upfront, encode_and_send, state)

        @pl.when(mx == 0)
        def _():
            pl.semaphore_wait(x_entered, 1)

        state = lax.fori_loop(upfront, Y_BLOCKS, encode_and_relay, state)
        encoded = 2 * (Y_BLOCKS - upfront)
        relay(encoded)
        for k, unit in enumerate(_close(state, reference)):
            tx[SUFFIX + k] = unit
        y_copy(SUFFIX).start()
        relay(encoded + 1)
        header = pl.ds(HEADER_ROW, 1)
        header_copy = pltpu.make_async_remote_copy(
            tx.at[POOL, header], x_header.at[header], header_sems.at[0],
            header_sems.at[1], x_nbr, MESH)
        header_copy.start()

        for u in range(SUFFIX + 1, PACED):
            y_copy(u).start()

        @pl.loop(encoded + 2, BACKLOG_START)
        def _(u):
            relay(u)
            v = PACED + 2 * (u - encoded - 2)

            @pl.when(v < Y_UNITS)
            def _():
                y_copy(v).start()
                y_copy(v + 1).start()

        def receiver(buf, sender_mx):
            state, reference = _reopen([buf[SUFFIX + k] for k in range(OWN)],
                                       lambda i: buf[POOL, pl.ds(i, 1)])
            both, each = _offsets(reference)

            def exponents(codes, j, state, first=False):
                t, state = _decode(_shr(codes, 2 * j) & _bytes(3), state)
                return _rotl(_where(first, t + each, t), 31), state

            def add(g, j, q, first=False):
                words = _join(buf[_frac_at(g, j)], q)
                words = [_where(first, w ^ flip, both - w) for w in words]
                other = pltpu.bitcast(jnp.concatenate(words, axis=1), jnp.bfloat16)
                window = piece(g, j, sender_mx)
                total = xs[window] + other.astype(jnp.float32)
                out[window] = total.astype(out.dtype)

            return state, exponents, add

        y_state, y_exponents, y_add = receiver(ry, mx)

        def decode_backlog(g, carry):
            u, state = carry
            codes, qs = ry[_code_at(g)], []
            for j in range(4):
                q, state = y_exponents(codes, j, state, g == 0)
                qs.append(q)
                if j % 2:
                    relay(u + j // 2)
                    y_add(g, j - 1, qs[j - 1], g == 0)
                    y_add(g, j, qs[j], g == 0)
            spare = lax.rem(g, 3) == 2
            pl.when(spare)(lambda: relay(u + 2))
            return u + 2 + spare.astype(jnp.int32), state

        _, y_state = lax.fori_loop(0, BACKLOG, decode_backlog,
                                   (BACKLOG_START, y_state))

        pltpu.make_async_copy(landed, landed, x_recv.at[0]).wait()
        load_rest.wait()
        x_state, x_exponents, x_add = receiver(rx, 1 - mx)

        def decode_round(relaying, k, states):
            y_state, x_state = states
            g = BACKLOG + k
            first = [k == 0 if relaying else False, False]
            x_codes, x_qs = [rx[_code_at(2 * k)]], []
            for step, pieces in enumerate(((0,), (1, 2), (3, 4), (5, 6), (7,), ())):
                if step > 0:
                    u = ROUNDS_START + 5 * k + step - 1
                    y_copy(u).wait_recv()
                    if relaying:
                        x_copy(u).start()
                    x_copy(u - X_LAG).wait_recv()
                if step == 1:
                    y_codes = ry[_code_at(g)]
                    x_codes.append(rx[_code_at(2 * k + 1)])
                if step > 1:
                    y_add(g, step - 2, y_q)
                for i, q in x_qs:
                    x_add(2 * k + i // 4, i % 4, q, first[i // 4])
                if 0 < step < 5:
                    y_q, y_state = y_exponents(y_codes, step - 1, y_state)
                x_qs = []
                for i in pieces:
                    q, x_state = x_exponents(x_codes[i // 4], i % 4, x_state,
                                             first[i // 4])
                    x_qs.append((i, q))
            return y_state, x_state

        relayed = X_BLOCKS - BACKLOG
        states = lax.fori_loop(0, relayed, functools.partial(decode_round, True),
                               (y_state, x_state))
        header_copy.wait()
        flags = (tx[POOL, header] | ry[POOL, header] | rx[POOL, header]
                 | x_header[header])
        misfit = jnp.max((flags & MISFIT).astype(jnp.float32)) > 0
        lax.fori_loop(relayed, ROUNDS, functools.partial(decode_round, False),
                      states)
        for sent, sem in ((tx, y_send), (ry.at[pl.ds(0, X_UNITS)], x_send)):
            pltpu.make_async_copy(sent, sent, sem).wait()

        @pl.when(misfit)
        def _plain_bfloat16_exchange():
            def rows(i):
                row = (mx * RAW_CHUNKS + i) * RAW_ROWS % M
                return pl.ds(pl.multiple_of(row, RAW_ROWS), RAW_ROWS)

            def raw_copy(i):
                return pltpu.make_async_remote_copy(
                    raw_tx.at[i], raw_rx.at[i], raw_sems.at[0],
                    raw_sems.at[3 + i], y_nbr, MESH)

            @pl.loop(0, RAW_CHUNKS)
            def _(i):
                raw_tx[i] = xs[rows(i)].astype(jnp.bfloat16)
                raw_copy(i).start()

            @pl.loop(0, RAW_CHUNKS)
            def _(i):
                raw_copy(i).wait_recv()
                pltpu.make_async_remote_copy(
                    raw_rx.at[i], raw_rx.at[RAW_CHUNKS + i], raw_sems.at[1],
                    raw_sems.at[2], x_nbr, MESH).start()

            for k, moved in enumerate((raw_tx, raw_rx.at[pl.ds(0, RAW_CHUNKS)],
                                       raw_rx.at[pl.ds(RAW_CHUNKS, RAW_CHUNKS)])):
                pltpu.make_async_copy(moved, moved, raw_sems.at[k]).wait()

            @pl.loop(0, 2 * RAW_CHUNKS)
            def _(i):
                total = xs[rows(i)] + raw_rx[i].astype(jnp.float32)
                out[rows(i)] = total.astype(out.dtype)

    return pl.pallas_call(
        kernel_body,
        out_shape=jax.ShapeDtypeStruct((M, N), jnp.bfloat16),
        in_specs=[pl.BlockSpec(memory_space=pltpu.HBM)],
        out_specs=pl.BlockSpec(memory_space=pltpu.VMEM),
        scratch_shapes=[
            pltpu.VMEM((M, N), jnp.float32),
            pltpu.VMEM((Y_UNITS, *VREG), jnp.int32),
            pltpu.VMEM((Y_UNITS, *VREG), jnp.int32),
            pltpu.VMEM((X_UNITS, *VREG), jnp.int32),
            pltpu.VMEM(VREG, jnp.int32),
            pltpu.VMEM((RAW_CHUNKS, RAW_ROWS, N), jnp.bfloat16),
            pltpu.VMEM((2 * RAW_CHUNKS, RAW_ROWS, N), jnp.bfloat16),
            pltpu.SemaphoreType.DMA((Y_BLOCKS + 4,)),
            pltpu.SemaphoreType.DMA,
            pltpu.SemaphoreType.DMA((Y_UNITS,)),
            pltpu.SemaphoreType.DMA,
            pltpu.SemaphoreType.DMA((5 * ROUNDS + 1,)),
            pltpu.SemaphoreType.DMA((2,)),
            pltpu.SemaphoreType.DMA((3 + RAW_CHUNKS,)),
            pltpu.SemaphoreType.REGULAR,
        ],
        compiler_params=pltpu.CompilerParams(
            collective_id=0,
            disable_bounds_checks=True,
            disable_semaphore_checks=True,
        ),
    )(x)
```
